```python
import numpy as np

kernel_name = "dist_sum_ax0_shard0_i_m1536_n768"

def setup_inputs():
    return {"x": np.random.randn(6144, 768).astype(np.float32)}

def reference(x: np.ndarray) -> np.ndarray:
    return np.sum(x, axis=0, keepdims=True)
```

```python
import jax
import jax.numpy as jnp
from jax import lax
from jax.experimental import pallas as pl
from jax.experimental.pallas import tpu as pltpu

N_DEV = 4
N_CHUNKS = 8


def pallas_dist_sum_ax0_shard0_i_m1536_n768_kernel(
x: jax.Array,
):
    m, n = x.shape
    rows = m // N_CHUNKS

    def body(x_hbm, out_ref, xbuf, comm_buf, in_sems, send_sems, recv_sems):
        my = lax.axis_index("i")

        copies = []
        for c in range(N_CHUNKS):
            cp = pltpu.make_async_copy(
                x_hbm.at[pl.ds(c * rows, rows)],
                xbuf.at[pl.ds(c * rows, rows)],
                in_sems.at[c],
            )
            cp.start()
            copies.append(cp)

        bar = pltpu.get_barrier_semaphore()
        for d in range(1, N_DEV):
            pl.semaphore_signal(
                bar, inc=1, device_id=((my + d) % N_DEV,),
                device_id_type=pl.DeviceIdType.MESH)

        acc = jnp.zeros((8, n), jnp.float32)
        for c in range(N_CHUNKS):
            copies[c].wait()
            blk = xbuf[pl.ds(c * rows, rows), :]
            acc = acc + blk.reshape(rows // 8, 8, n).sum(axis=0)
        comm_buf[my] = acc.sum(axis=0, keepdims=True)

        pl.semaphore_wait(bar, N_DEV - 1)
        rdmas = []
        for k, d in enumerate((2, 1, 3)):
            r = pltpu.make_async_remote_copy(
                src_ref=comm_buf.at[my], dst_ref=comm_buf.at[my],
                send_sem=send_sems.at[k], recv_sem=recv_sems.at[d - 1],
                device_id=((my + d) % N_DEV,),
                device_id_type=pl.DeviceIdType.MESH)
            r.start()
            rdmas.append(r)
        for r in rdmas:
            r.wait_recv()
        out_ref[...] = (comm_buf[0] + comm_buf[1]) + (comm_buf[2] + comm_buf[3])
        for r in rdmas:
            r.wait_send()

    return pl.pallas_call(
        body,
        out_shape=jax.ShapeDtypeStruct((1, n), jnp.float32),
        in_specs=[pl.BlockSpec(memory_space=pl.ANY)],
        out_specs=pl.BlockSpec(memory_space=pltpu.VMEM),
        scratch_shapes=[
            pltpu.VMEM((m, n), jnp.float32),
            pltpu.VMEM((N_DEV, 1, n), jnp.float32),
            pltpu.SemaphoreType.DMA((N_CHUNKS,)),
            pltpu.SemaphoreType.DMA((N_DEV - 1,)),
            pltpu.SemaphoreType.DMA((N_DEV - 1,)),
        ],
        compiler_params=pltpu.CompilerParams(
            collective_id=0,
            disable_bounds_checks=True,
            disable_semaphore_checks=True,
        ),
    )(x)
```

```python
import jax
import jax.numpy as jnp
from jax import lax
from jax.experimental import pallas as pl
from jax.experimental.pallas import tpu as pltpu

N_DEV = 4
LANES = 128
SUBLANES = 8

FULL_PIECES = (192, 192, 192, 192, 192, 192, 128)
B_PIECES = (192, 48, 16)
TAIL_ROWS = sum(B_PIECES)


def _tree_add(parts):
    while len(parts) > 1:
        nxt = [parts[i] + parts[i + 1] for i in range(0, len(parts) - 1, 2)]
        if len(parts) % 2:
            nxt.append(parts[-1])
        parts = nxt
    return parts[0]


def _fold_rows(blk, chains):
    rows, cols = blk.shape
    groups = rows // SUBLANES
    if chains == 1:
        return blk.reshape(groups, SUBLANES, cols).sum(axis=0)
    if groups % chains or groups < 2 * chains:
        v = blk.reshape(groups, SUBLANES, cols)
        return _tree_add([v[i] for i in range(groups)])
    v = blk.reshape(chains, groups // chains, SUBLANES, cols).sum(axis=1)
    return _tree_add([v[i] for i in range(chains)])


def pallas_dist_sum_ax0_shard0_i_m1536_n768_kernel(
x: jax.Array,
):
    m, n = x.shape
    wb = LANES
    wa = n - wb
    tail0 = sum(FULL_PIECES)
    assert tail0 + TAIL_ROWS == m

    pieces = []
    row = 0
    for rows in FULL_PIECES:
        pieces.append((row, rows, 0, n))
        row += rows
    pieces.append((tail0, TAIL_ROWS, 0, wa))
    last_a = len(pieces) - 1
    row = tail0
    for rows in B_PIECES:
        pieces.append((row, rows, wa, wb))
        row += rows

    def body(x_hbm, out_ref, xbuf, send_a, send_b, recv_a, recv_b,
             in_sems, send_sems, recv_sems):
        copies = []
        for k, (r0, rows, c0, cols) in enumerate(pieces):
            if cols == n:
                window = (pl.ds(r0, rows),)
            else:
                window = (pl.ds(r0, rows), pl.ds(c0, cols))
            cp = pltpu.make_async_copy(
                x_hbm.at[window], xbuf.at[window], in_sems.at[k])
            cp.start()
            copies.append(cp)

        my = lax.axis_index("i")

        def peer(d):
            return dict(device_id=((my + d) & (N_DEV - 1),),
                        device_id_type=pl.DeviceIdType.MESH)

        bar = pltpu.get_barrier_semaphore()
        for d in range(1, N_DEV):
            pl.semaphore_signal(bar, inc=1, **peer(d))

        def broadcast(src, dst, sem0):
            rdmas = {}
            for d in (2, 1, 3):
                rdmas[d] = pltpu.make_async_remote_copy(
                    src_ref=src, dst_ref=dst.at[d - 1],
                    send_sem=send_sems.at[sem0 + d - 1],
                    recv_sem=recv_sems.at[sem0 + d - 1], **peer(d))
                rdmas[d].start()
            return rdmas

        acc_a = jnp.zeros((SUBLANES, wa), jnp.float32)
        acc_b = jnp.zeros((SUBLANES, wb), jnp.float32)
        for k, (r0, rows, c0, cols) in enumerate(pieces):
            copies[k].wait()
            if k == 0:
                pl.semaphore_wait(bar, N_DEV - 1)
            blk = xbuf[pl.ds(r0, rows), pl.ds(c0, cols)]
            if cols == n:
                s = _fold_rows(blk, 1)
                acc_a = acc_a + s[:, :wa]
                acc_b = acc_b + s[:, wa:]
            elif cols == wa:
                acc_a = acc_a + _fold_rows(blk, 1)
            else:
                acc_b = acc_b + _fold_rows(blk, 8)
            if k == last_a:
                part_a = acc_a.sum(axis=0, keepdims=True)
                send_a[...] = part_a
                rd_a = broadcast(send_a, recv_a, 0)

        part_b = acc_b.sum(axis=0, keepdims=True)
        send_b[...] = part_b
        rd_b = broadcast(send_b, recv_b, N_DEV - 1)

        for d in (1, 3):
            rd_a[d].wait_recv()
            rd_b[d].wait_recv()
        near_a = recv_a[0] + recv_a[2]
        near_b = recv_b[0] + recv_b[2]
        for d in (1, 3, 2):
            rd_a[d].wait_send()
            rd_b[d].wait_send()
        rd_a[2].wait_recv()
        out_ref[:, :wa] = (part_a + recv_a[1]) + near_a
        rd_b[2].wait_recv()
        out_ref[:, wa:] = (part_b + recv_b[1]) + near_b

    return pl.pallas_call(
        body,
        out_shape=jax.ShapeDtypeStruct((1, n), jnp.float32),
        in_specs=[pl.BlockSpec(memory_space=pl.ANY)],
        out_specs=pl.BlockSpec(memory_space=pltpu.VMEM),
        scratch_shapes=[
            pltpu.VMEM((m, n), jnp.float32),
            pltpu.VMEM((1, wa), jnp.float32),
            pltpu.VMEM((1, wb), jnp.float32),
            pltpu.VMEM((N_DEV - 1, 1, wa), jnp.float32),
            pltpu.VMEM((N_DEV - 1, 1, wb), jnp.float32),
            pltpu.SemaphoreType.DMA((len(pieces),)),
            pltpu.SemaphoreType.DMA((2 * (N_DEV - 1),)),
            pltpu.SemaphoreType.DMA((2 * (N_DEV - 1),)),
        ],
        compiler_params=pltpu.CompilerParams(
            collective_id=0,
            disable_bounds_checks=True,
            disable_semaphore_checks=True,
        ),
    )(x)
```

```python
import jax
import jax.numpy as jnp
from jax import lax
from jax.experimental import pallas as pl
from jax.experimental.pallas import tpu as pltpu

N_DEV = 4
LANES = 128
SUBLANES = 8

FULL_PIECES = (192, 192, 192, 192, 192, 192, 64)
A_PIECES = (288, 32)
B_PIECES = (256, 48, 16)


def _tree_add(parts):
    while len(parts) > 1:
        nxt = [parts[i] + parts[i + 1] for i in range(0, len(parts) - 1, 2)]
        if len(parts) % 2:
            nxt.append(parts[-1])
        parts = nxt
    return parts[0]


def _fold_rows(blk, chains):
    rows, cols = blk.shape
    groups = rows // SUBLANES
    if chains == 1:
        return blk.reshape(groups, SUBLANES, cols).sum(axis=0)
    if groups % chains or groups < 2 * chains:
        v = blk.reshape(groups, SUBLANES, cols)
        return _tree_add([v[i] for i in range(groups)])
    v = blk.reshape(chains, groups // chains, SUBLANES, cols).sum(axis=1)
    return _tree_add([v[i] for i in range(chains)])


def pallas_dist_sum_ax0_shard0_i_m1536_n768_kernel(
x: jax.Array,
):
    m, n = x.shape
    wb = LANES
    wa = n - wb
    tail0 = sum(FULL_PIECES)
    assert tail0 + sum(A_PIECES) == m and tail0 + sum(B_PIECES) == m

    pieces = []
    row = 0
    for rows in FULL_PIECES:
        pieces.append((row, rows, 0, n))
        row += rows
    row = tail0
    for rows in A_PIECES:
        pieces.append((row, rows, 0, wa))
        row += rows
    last_a = len(pieces) - 1
    row = tail0
    for rows in B_PIECES:
        pieces.append((row, rows, wa, wb))
        row += rows

    def body(x_hbm, out_ref, xbuf, send_a, send_b, send_full,
             diag_a, diag_b, near, in_sems, send_sems, recv_sems):
        copies = []
        for k, (r0, rows, c0, cols) in enumerate(pieces):
            if cols == n:
                window = (pl.ds(r0, rows),)
            else:
                window = (pl.ds(r0, rows), pl.ds(c0, cols))
            cp = pltpu.make_async_copy(
                x_hbm.at[window], xbuf.at[window], in_sems.at[k])
            cp.start()
            copies.append(cp)

        my = lax.axis_index("i")

        def peer(d):
            return dict(device_id=((my + d) & (N_DEV - 1),),
                        device_id_type=pl.DeviceIdType.MESH)

        bar = pltpu.get_barrier_semaphore()
        for d in range(1, N_DEV):
            pl.semaphore_signal(bar, inc=1, **peer(d))

        def send(src, dst, sem, d):
            rdma = pltpu.make_async_remote_copy(
                src_ref=src, dst_ref=dst, send_sem=send_sems.at[sem],
                recv_sem=recv_sems.at[sem], **peer(d))
            rdma.start()
            return rdma

        acc_a = jnp.zeros((SUBLANES, wa), jnp.float32)
        acc_b = jnp.zeros((SUBLANES, wb), jnp.float32)
        for k, (r0, rows, c0, cols) in enumerate(pieces):
            copies[k].wait()
            if k == 0:
                pl.semaphore_wait(bar, N_DEV - 1)
            blk = xbuf[pl.ds(r0, rows), pl.ds(c0, cols)]
            if cols == n:
                s = _fold_rows(blk, 1)
                acc_a = acc_a + s[:, :wa]
                acc_b = acc_b + s[:, wa:]
            elif cols == wa:
                acc_a = acc_a + _fold_rows(blk, 1)
            else:
                acc_b = acc_b + _fold_rows(blk, 8)
            if k == last_a:
                part_a = acc_a.sum(axis=0, keepdims=True)
                send_a[...] = part_a
                to_diag_a = send(send_a, diag_a, 0, 2)
                send_full[:, :wa] = part_a

        part_b = acc_b.sum(axis=0, keepdims=True)
        send_b[...] = part_b
        to_diag_b = send(send_b, diag_b, 1, 2)

        send_full[:, wa:] = part_b
        to_near = [send(send_full, near.at[0], 2, 1),
                   send(send_full, near.at[1], 3, 3)]

        for rdma in to_near:
            rdma.wait_recv()
        rest = (near[0] + near[1]) + send_full[...]
        for rdma in to_near + [to_diag_a, to_diag_b]:
            rdma.wait_send()
        to_diag_a.wait_recv()
        out_ref[:, :wa] = rest[:, :wa] + diag_a[...]
        to_diag_b.wait_recv()
        out_ref[:, wa:] = rest[:, wa:] + diag_b[...]

    return pl.pallas_call(
        body,
        out_shape=jax.ShapeDtypeStruct((1, n), jnp.float32),
        in_specs=[pl.BlockSpec(memory_space=pl.ANY)],
        out_specs=pl.BlockSpec(memory_space=pltpu.VMEM),
        scratch_shapes=[
            pltpu.VMEM((m, n), jnp.float32),
            pltpu.VMEM((1, wa), jnp.float32),
            pltpu.VMEM((1, wb), jnp.float32),
            pltpu.VMEM((1, n), jnp.float32),
            pltpu.VMEM((1, wa), jnp.float32),
            pltpu.VMEM((1, wb), jnp.float32),
            pltpu.VMEM((2, 1, n), jnp.float32),
            pltpu.SemaphoreType.DMA((len(pieces),)),
            pltpu.SemaphoreType.DMA((4,)),
            pltpu.SemaphoreType.DMA((4,)),
        ],
        compiler_params=pltpu.CompilerParams(
            collective_id=0,
            disable_bounds_checks=True,
            disable_semaphore_checks=True,
        ),
    )(x)
```

```python
import jax
import jax.numpy as jnp
from jax import lax
from jax.experimental import pallas as pl
from jax.experimental.pallas import tpu as pltpu

N_DEV = 4
LANES = 128
SUBLANES = 8

LATE = 2

FULL_PIECES = (192, 192, 192, 192, 192, 192, 64)
PUSH_ROWS = 88
C_PIECES = (112, 32)
B_PIECES = (256, 48, 16)


def _tree_add(parts):
    while len(parts) > 1:
        nxt = [parts[i] + parts[i + 1] for i in range(0, len(parts) - 1, 2)]
        if len(parts) % 2:
            nxt.append(parts[-1])
        parts = nxt
    return parts[0]


def _fold_rows(blk, chains):
    rows, cols = blk.shape
    groups = rows // SUBLANES
    if chains == 1:
        return blk.reshape(groups, SUBLANES, cols).sum(axis=0)
    if groups % chains or groups < 2 * chains:
        v = blk.reshape(groups, SUBLANES, cols)
        return _tree_add([v[i] for i in range(groups)])
    v = blk.reshape(chains, groups // chains, SUBLANES, cols).sum(axis=1)
    return _tree_add([v[i] for i in range(chains)])


def pallas_dist_sum_ax0_shard0_i_m1536_n768_kernel(
x: jax.Array,
):
    m, n = x.shape
    wb = LANES
    wc = n - wb
    tail0 = sum(FULL_PIECES)
    assert tail0 + 2 * PUSH_ROWS + sum(C_PIECES) == m
    assert tail0 + sum(B_PIECES) == m

    pieces = []

    def add_pieces(row, sizes, col0, cols):
        ids = []
        for rows in sizes:
            ids.append(len(pieces))
            pieces.append((row, rows, col0, cols))
            row += rows
        return ids

    full_ids = add_pieces(0, FULL_PIECES, 0, n)
    push_ids = add_pieces(tail0, (2 * PUSH_ROWS,), 0, wc)
    c_ids = add_pieces(tail0 + 2 * PUSH_ROWS, C_PIECES, 0, wc)
    b_ids = add_pieces(tail0, B_PIECES, wc, wb)

    def body(x_hbm, out_ref, xbuf, raw, send_b, got_b, send_c, got_c, send_f,
             in_sems, send_b_sem, recv_b_sems, send_c_sems, recv_c_sems,
             send_f_sems, recv_f_sem, send_raw_sems, recv_raw_sem):
        copies = []
        for k, (r0, rows, c0, cols) in enumerate(pieces):
            if cols == n:
                window = (pl.ds(r0, rows),)
            else:
                window = (pl.ds(r0, rows), pl.ds(c0, cols))
            copies.append(pltpu.make_async_copy(
                x_hbm.at[window], xbuf.at[window], in_sems.at[k]))

        for k in full_ids:
            copies[k].start()

        my = lax.axis_index("i")
        is_late = my == LATE
        is_early = jnp.logical_not(is_late)

        @pl.when(is_late)
        def _():
            for k in c_ids + b_ids:
                copies[k].start()

        @pl.when(is_early)
        def _():
            for k in b_ids + push_ids + c_ids:
                copies[k].start()

        def peer(d):
            return dict(device_id=((my + d) & (N_DEV - 1),),
                        device_id_type=pl.DeviceIdType.MESH)

        bar = pltpu.get_barrier_semaphore()
        for d in range(1, N_DEV):
            pl.semaphore_signal(bar, inc=1, **peer(d))
        pl.semaphore_wait(bar, N_DEV - 1)

        to_raw = [
            pltpu.make_async_remote_copy(
                src_ref=x_hbm.at[pl.ds(tail0 + j * PUSH_ROWS, PUSH_ROWS),
                                 pl.ds(0, wc)],
                dst_ref=raw, send_sem=send_raw_sems.at[j],
                recv_sem=recv_raw_sem, **peer(d))
            for j, d in enumerate((1, 3))]

        @pl.when(is_late)
        def _():
            for rdma in to_raw:
                rdma.start()

        def fold(k):
            r0, rows, c0, cols = pieces[k]
            copies[k].wait()
            blk = xbuf[pl.ds(r0, rows), pl.ds(c0, cols)]
            return _fold_rows(blk, 8 if cols == wb else 1)

        full_c = jnp.zeros((SUBLANES, wc), jnp.float32)
        full_b = jnp.zeros((SUBLANES, wb), jnp.float32)
        for k in full_ids:
            s = fold(k)
            full_c = full_c + s[:, :wc]
            full_b = full_b + s[:, wc:]

        to_c = [
            pltpu.make_async_remote_copy(
                src_ref=send_c, dst_ref=got_c.at[d - 1],
                send_sem=send_c_sems.at[d - 1],
                recv_sem=recv_c_sems.at[d - 1], **peer(d))
            for d in range(1, N_DEV)]
        to_f = [
            pltpu.make_async_remote_copy(
                src_ref=send_f, dst_ref=out_ref.at[:, pl.ds(wc, wb)],
                send_sem=send_f_sems.at[d - 1], recv_sem=recv_f_sem,
                **peer(d))
            for d in range(1, N_DEV)]

        def to_late_b(slot):
            return pltpu.make_async_remote_copy(
                src_ref=send_b, dst_ref=got_b.at[slot], send_sem=send_b_sem,
                recv_sem=recv_b_sems.at[slot], device_id=(LATE,),
                device_id_type=pl.DeviceIdType.MESH)

        def finish_c():
            for rdma in to_c:
                rdma.wait_recv()
            out_ref[:, pl.ds(0, wc)] = ((got_c[0] + got_c[1])
                                        + (got_c[2] + send_c[...]))

        @pl.when(is_late)
        def _():
            acc_c, acc_b = full_c, full_b
            for k in c_ids:
                acc_c = acc_c + fold(k)
            send_c[...] = acc_c.sum(axis=0, keepdims=True)
            for d in (2, 1, 3):
                to_c[d - 1].start()

            for slot in range(N_DEV - 1):
                to_late_b(slot).wait_recv()
            acc_b = acc_b + ((got_b[0] + got_b[1]) + got_b[2])
            for k in b_ids:
                acc_b = acc_b + fold(k)
            total_b = acc_b.sum(axis=0, keepdims=True)
            send_f[...] = total_b
            for d in (2, 1, 3):
                to_f[d - 1].start()
            out_ref[:, pl.ds(wc, wb)] = total_b

            finish_c()
            for rdma in to_c + to_f + to_raw:
                rdma.wait_send()

        @pl.when(is_early)
        def _():
            acc_c, acc_b = full_c, full_b
            for k in b_ids:
                acc_b = acc_b + fold(k)
            send_b[...] = acc_b
            to_b = to_late_b(((my - LATE) & (N_DEV - 1)) - 1)
            to_b.start()

            for k in push_ids + c_ids:
                acc_c = acc_c + fold(k)

            def add_raw(acc):
                to_raw[0].wait_recv()
                return acc + _fold_rows(raw[...], 1)

            is_neighbour = ((my - LATE) & 1) == 1
            acc_c = lax.cond(is_neighbour, add_raw, lambda acc: acc, acc_c)
            send_c[...] = acc_c.sum(axis=0, keepdims=True)
            for d in (1, 3, 2):
                to_c[d - 1].start()

            for rdma in to_c + [to_b]:
                rdma.wait_send()
            finish_c()
            to_f[0].wait_recv()

    return pl.pallas_call(
        body,
        out_shape=jax.ShapeDtypeStruct((1, n), jnp.float32),
        in_specs=[pl.BlockSpec(memory_space=pl.ANY)],
        out_specs=pl.BlockSpec(memory_space=pltpu.VMEM),
        scratch_shapes=[
            pltpu.VMEM((m, n), jnp.float32),
            pltpu.VMEM((PUSH_ROWS, wc), jnp.float32),
            pltpu.VMEM((SUBLANES, wb), jnp.float32),
            pltpu.VMEM((N_DEV - 1, SUBLANES, wb), jnp.float32),
            pltpu.VMEM((1, wc), jnp.float32),
            pltpu.VMEM((N_DEV - 1, 1, wc), jnp.float32),
            pltpu.VMEM((1, wb), jnp.float32),
            pltpu.SemaphoreType.DMA((len(pieces),)),
            pltpu.SemaphoreType.DMA,
            pltpu.SemaphoreType.DMA((N_DEV - 1,)),
            pltpu.SemaphoreType.DMA((N_DEV - 1,)),
            pltpu.SemaphoreType.DMA((N_DEV - 1,)),
            pltpu.SemaphoreType.DMA((N_DEV - 1,)),
            pltpu.SemaphoreType.DMA,
            pltpu.SemaphoreType.DMA((2,)),
            pltpu.SemaphoreType.DMA,
        ],
        compiler_params=pltpu.CompilerParams(
            collective_id=0,
            disable_bounds_checks=True,
            disable_semaphore_checks=True,
        ),
    )(x)
```
